```python
import numpy as np

kernel_name = "dist_rope_attn_qseq_b2_sq128_d512_hq4_dh64"

def setup_inputs():
    x = np.random.randn(2, 512, 512).astype(np.float32)
    Wq = np.random.randn(512, 256).astype(np.float32) * 0.02
    Wk = np.random.randn(512, 256).astype(np.float32) * 0.02
    Wv = np.random.randn(512, 256).astype(np.float32) * 0.02
    Wo = np.random.randn(256, 512).astype(np.float32) * 0.02
    return {"x": x, "Wq": Wq, "Wk": Wk, "Wv": Wv, "Wo": Wo}

def reference(x, Wq, Wk, Wv, Wo):
    B, Sq, Hq, Dh = 2, 512, 4, 64
    inv = 1.0 / (10000.0 ** (np.arange(0, Dh, 2) / Dh))
    pos = np.arange(Sq)[:, None] * inv[None, :]
    cos = np.repeat(np.cos(pos), 2, axis=-1).astype(np.float32)
    sin = np.repeat(np.sin(pos), 2, axis=-1).astype(np.float32)
    def rot(t):
        t2 = t.reshape(B, Sq, Hq, Dh // 2, 2)
        t_r = np.stack([-t2[..., 1], t2[..., 0]], axis=-1).reshape(B, Sq, Hq, Dh)
        return t * cos[None, :, None, :] + t_r * sin[None, :, None, :]
    Q = rot((x @ Wq).reshape(B, Sq, Hq, Dh))
    K = rot((x @ Wk).reshape(B, Sq, Hq, Dh))
    V = (x @ Wv).reshape(B, Sq, Hq, Dh)
    s = np.einsum('bihd,bjhd->bhij', Q, K).astype(np.float32) * 0.125
    s_max = s.max(axis=-1, keepdims=True)
    w = np.exp(s - s_max)
    w = w / w.sum(axis=-1, keepdims=True)
    ctx = np.einsum('bhij,bjhd->bihd', w, V).reshape(B, Sq, Hq * Dh)
    return ctx @ Wo
```

```python
import functools

import numpy as np
import jax
import jax.numpy as jnp
from jax import lax
from jax.experimental import pallas as pl
from jax.experimental.pallas import tpu as pltpu

BF = jnp.bfloat16
F32 = jnp.float32
U32 = jnp.uint32
MESH = pl.DeviceIdType.MESH
LOG2E = 1.4426950408889634
Q_SCALE = 0.125 * LOG2E
NEG_LOG_BASE = float(-np.log(10000.0) / 32.0)

LOADS = ("x0", "x1", "k0", "k1", "v0", "v1", "q0", "q1", "o0", "o1")

SCHEDULE = """
v1 x0 q0 x1 k1 k0 v0 q1 o0 o1 | p_v_3 tab barw s_v_3 p_v_1 s_v_1 p_k_3 s_k_3 p_q_2 p_k_1 s_k_1 p_v_2 p_v_0 dgw s_q_2 p_q_3 p_k_2 s_k_2 s_v_2 p_q_0 p_q_1 p_k_0 s_q_1 woc s_q_3 A_0 op_0 A_1 so_1 A_3 so_3 A_2 so_2 op_1 op_3 op_2
v0 x1 v1 k0 x0 k1 q0 q1 o0 o1 | tab p_v_2 barw s_v_2 p_v_1 s_v_1 p_k_2 s_k_2 p_k_3 p_v_3 f s_k_3 p_q_0 s_v_3 p_k_0 f p_k_1 p_v_0 s_k_1 p_q_1 p_q_2 s_q_2 p_q_3 s_q_3 s_q_1 S_0 PV_0 so_0 A_3 so_3 S_1 A_2 woc so_2 PV_1 op_1 op_0 op_3 op_2
v0 x1 k0 k1 x0 q0 v1 q1 o0 o1 | barw tab p_v_2 s_v_2 p_k_2 s_k_2 p_k_1 f p_k_3 s_k_1 s_k_3 p_k_0 f p_q_0 p_v_1 p_v_3 s_v_3 p_q_2 s_v_1 s_q_2 p_q_1 p_v_0 p_q_3 s_q_3 f S_0 woc s_q_1 PV_0 so_0 A_3 so_3 A_1 so_1 S_2 PV_2 op_1 op_0 op_3 op_2
x1 k1 k0 v1 v0 x0 q0 q1 o0 o1 | tab p_k_1 barw s_k_1 p_k_2 s_k_2 p_v_1 s_v_1 p_v_2 s_v_2 p_v_3 p_k_3 s_v_3 p_q_3 s_k_3 p_q_1 woc p_q_2 s_q_2 p_k_0 s_q_3 p_v_0 p_q_0 s_q_1 A_0 so_0 A_1 so_1 A_2 so_2 S_3 PV_3 op_1 op_0 op_3 op_2
"""
BRANCH_ORDER = (1, 2, 3, 0)


def _parse_schedule(text):
    loads, progs = [], []
    for line in text.strip().split("\n"):
        first, second = line.split("|")
        loads.append(tuple(first.split()))
        prog = []
        for tok in second.split():
            part = tok.split("_")
            if len(part) == 3:
                prog.append((part[0], part[1], int(part[2])))
            elif len(part) == 2:
                prog.append((part[0], int(part[1])))
            else:
                prog.append((part[0],))
        progs.append(tuple(prog))
    return tuple(loads), tuple(progs)


def _check_schedule(loads, progs):
    for me in range(4):
        prog = progs[me]
        assert sorted(loads[me]) == sorted(LOADS)
        for tensor in "kvq":
            for d in range(4):
                assert prog.count(("p", tensor, d)) == 1
                assert prog.count(("s", tensor, d)) == (1 if d else 0)
                if d:
                    assert prog.index(("p", tensor, d)) < prog.index(("s", tensor, d))
                    assert prog.index(("barw",)) < prog.index(("s", tensor, d))
            if me == 0:
                assert prog.index(("dgw",)) < prog.index(("s", tensor, 2))
            if tensor != "v":
                assert all(prog.index(("tab",)) < prog.index(("p", tensor, d)) for d in range(4))
        for i in range(4):
            whole = prog.count(("A", i))
            assert whole + prog.count(("S", i)) == 1 and whole + prog.count(("PV", i)) == 1
            first = prog.index(("A", i) if whole else ("S", i))
            last = prog.index(("A", i) if whole else ("PV", i))
            assert first <= last
            assert prog.index(("p", "k", 0)) < first and prog.index(("p", "v", 0)) < last
            if i == me:
                assert prog.index(("p", "q", 0)) < first and prog.count(("so", i)) == 0
                assert last < prog.index(("op", 0))
            else:
                assert prog.count(("so", i)) == 1 and last < prog.index(("so", i))
        for d in range(4):
            assert prog.count(("op", d)) == 1 and prog.index(("woc",)) < prog.index(("op", d))
        assert prog.count(("barw",)) == 1 and prog.count(("woc",)) == 1
        assert prog.count(("dgw",)) == (1 if me == 0 else 0)
        trailing = len(prog)
        while prog[trailing - 1][0] == "op":
            trailing -= 1
        assert all(("op", d) in prog[trailing:] for d in (1, 2, 3))


LOAD_ORDER, PROGRAMS = _parse_schedule(SCHEDULE)
_check_schedule(LOAD_ORDER, PROGRAMS)


def _parity(v):
    return ((v >> 1) ^ v) & 1


def _batch_slot(d):
    return _parity(d)


def _head_slot(d):
    return d & 1


SEM_BASE = {"k": 0, "v": 3, "q": 6, "o": 9}


def _sem(tensor, d):
    return SEM_BASE[tensor] + d - 1


def _body(x_hbm, wq_hbm, wk_hbm, wv_hbm, wo_hbm, o_ref,
          xs, wq, wk, wv, wo, sk, sv, sq, so, rk, rv, rq, ro, wob, pbuf, lbuf, tab,
          lsem, ssem, rsem, dsem):
    me_dyn = lax.axis_index("i")
    barrier = pltpu.get_barrier_semaphore()
    send_buf = {"k": sk, "v": sv, "q": sq, "o": so}

    def pack(t):
        return pltpu.bitcast(t.astype(BF), U32)

    def unpack(t):
        return pltpu.bitcast(t, BF)

    def left_half(rows):
        return lax.broadcasted_iota(jnp.int32, (rows, 128), 1) < 64

    def recv_buf(tensor, d):
        if tensor == "k":
            return rk.at[pl.ds(d * 64, 64)]
        if tensor == "v":
            return rv.at[pl.ds(d * 64, 64)]
        return (rq if tensor == "q" else ro).at[d]

    def remote(tensor, d, peer):
        return pltpu.make_async_remote_copy(
            send_buf[tensor].at[d], recv_buf(tensor, d),
            ssem.at[_sem(tensor, d)], rsem.at[_sem(tensor, d)],
            device_id=(peer,), device_id_type=MESH)

    def out_piece(ctx, w, batch):
        o_ref[batch] += jnp.dot(unpack(ctx), unpack(w), preferred_element_type=F32)

    tails = {}

    def program(me):
        prog = PROGRAMS[me]
        batch, hp = _parity(me), me & 1
        weights = {"k": (wk_hbm, wk), "v": (wv_hbm, wv), "q": (wq_hbm, wq)}

        loads = {}
        for n, name in enumerate(LOADS):
            slot = int(name[1])
            h = hp if slot == 0 else 1 - hp
            if name[0] == "x":
                src, dst = x_hbm.at[batch if slot == 0 else 1 - batch], xs.at[slot]
            elif name[0] == "o":
                src, dst = wo_hbm.at[pl.ds(h * 128, 128), :], wo.at[slot]
            else:
                src = weights[name[0]][0].at[:, pl.ds(h * 128, 128)]
                dst = weights[name[0]][1].at[slot]
            loads[name] = pltpu.make_async_copy(src, dst, lsem.at[n])
        for name in LOAD_ORDER[me]:
            loads[name].start()

        for d in ((1, 3) if me == 2 else (1, 2, 3)):
            pl.semaphore_signal(barrier, inc=1, device_id=(me ^ d,), device_id_type=MESH)
        barrier_count = 2 if me == 0 else 3

        landed = []

        def need(*names):
            for name in names:
                if name not in landed:
                    loads[name].wait()
                    landed.append(name)

        received = []

        def need_remote(tensor, d):
            if (tensor, d) not in received:
                remote(tensor, d, me ^ d).wait_recv()
                received.append((tensor, d))

        zeroed = []

        def zero_output():
            if not zeroed:
                o_ref[...] = jnp.zeros(o_ref.shape, F32)
                zeroed.append(True)

        def tables():
            row = lax.broadcasted_iota(jnp.int32, (128, 128), 0)
            lane = lax.broadcasted_iota(jnp.int32, (128, 128), 1)
            pos = (row + me * 128).astype(F32)
            freq = ((lane % 64) // 2).astype(F32)
            angle = pos * jnp.exp(freq * NEG_LOG_BASE)
            sin = jnp.sin(angle)
            tab[0] = jnp.cos(angle)
            tab[1] = jnp.where(lane % 2 == 0, -sin, sin)

        def rope(t):
            lane = lax.broadcasted_iota(jnp.int32, (128, 128), 1)
            partner = jnp.take_along_axis(t, jnp.bitwise_xor(lane, 1), axis=1)
            return t * tab[0] + partner * tab[1]

        def project(tensor, d):
            t = jnp.dot(xs[_batch_slot(d)].astype(BF),
                        weights[tensor][1][_head_slot(d)].astype(BF),
                        preferred_element_type=F32)
            if tensor == "k":
                t = rope(t)
            elif tensor == "q":
                t = rope(t) * Q_SCALE
            t = pack(t)
            if d:
                send_buf[tensor][d] = t
            elif tensor == "k":
                rk[pl.ds(0, 64)] = t
            elif tensor == "v":
                rv[pl.ds(0, 64)] = t
            else:
                rq[0] = t

        def stacked_q(d):
            q = rq[d]
            zero = jnp.zeros_like(q)
            left = left_half(64)
            return jnp.concatenate([jnp.where(left, q, zero), jnp.where(left, zero, q)], axis=0)

        def softmax_part(ds):
            q = unpack(jnp.concatenate([stacked_q(d) for d in ds], axis=0))
            s = lax.dot_general(q, unpack(rk[...]), (((1,), (1,)), ((), ())),
                                preferred_element_type=F32)
            p = jnp.exp2(s - jnp.max(s, axis=1, keepdims=True))
            return p.astype(BF), jnp.sum(p, axis=1, keepdims=True)

        def inverse(l):
            l = jnp.where(left_half(128), l[:128], l[128:])
            r = pl.reciprocal(l, approx=True)
            return r * (2.0 - l * r)

        def value_part(p):
            return jnp.dot(p, unpack(rv[...]), preferred_element_type=F32)

        def finish(r, inv):
            return pack(jnp.where(left_half(128), r[:128], r[128:]) * inv)

        n = len(prog)
        while prog[n - 1][0] == "op":
            n -= 1
        tails[me] = [step[1] for step in prog[n:]]

        at = 0
        while at < n:
            step = prog[at]
            group = [step]
            if step[0] in ("p", "A"):
                while at + len(group) < n and prog[at + len(group)][0] == step[0]:
                    group.append(prog[at + len(group)])
            at += len(group)
            kind = step[0]
            if kind == "p":
                for _, tensor, d in group:
                    need("x%d" % _batch_slot(d), "%s%d" % (tensor, _head_slot(d)))
                for _, tensor, d in group:
                    project(tensor, d)
            elif kind == "A":
                zero_output()
                ds = [me ^ g[1] for g in group]
                for d in (1, 2, 3):
                    need_remote("k", d)
                for d in ds:
                    if d:
                        need_remote("q", d)
                for d in (1, 2, 3):
                    need_remote("v", d)
                p, l = softmax_part(ds)
                r = value_part(p)
                for j, d in enumerate(ds):
                    rows = slice(256 * j, 256 * j + 256)
                    so[d] = finish(r[rows], inverse(l[rows]))
            elif kind == "S":
                zero_output()
                d = me ^ step[1]
                for dd in (1, 2, 3):
                    need_remote("k", dd)
                if d:
                    need_remote("q", d)
                p, l = softmax_part([d])
                pbuf[d] = pltpu.bitcast(p, U32)
                lbuf[d] = inverse(l)
            elif kind == "PV":
                d = me ^ step[1]
                for dd in (1, 2, 3):
                    need_remote("v", dd)
                so[d] = finish(value_part(unpack(pbuf[d])), lbuf[d])
            elif kind == "barw":
                pl.semaphore_wait(barrier, barrier_count)
                if me == 2:
                    pl.semaphore_signal(dsem, inc=1, device_id=(0,), device_id_type=MESH)
            elif kind == "dgw":
                pl.semaphore_wait(dsem, 1)
            elif kind == "tab":
                tables()
            elif kind == "s":
                remote(step[1], step[2], me ^ step[2]).start()
            elif kind == "so":
                d = me ^ step[1]
                remote("o", d, me ^ d).start()
            elif kind == "woc":
                need("o0", "o1")
                wob[0] = pack(wo[0])
                wob[1] = pack(wo[1])
            elif kind == "op":
                out_piece(so[0], wob[0], batch)
            else:
                assert kind == "f"
        need(*LOADS)

    for position in BRANCH_ORDER:
        pl.when(me_dyn == position)(functools.partial(program, position))

    def pick(values):
        if all(v == values[0] for v in values):
            return values[0]
        chosen = jnp.int32(values[3])
        for position in (2, 1, 0):
            chosen = jnp.where(me_dyn == position, values[position], chosen)
        return chosen

    def parity_dyn(v):
        return jnp.bitwise_and(jnp.bitwise_xor(v, v >> 1), 1)

    for tensor in "kvq":
        for d in (1, 2, 3):
            remote(tensor, d, me_dyn).wait_send()

    def own_piece():
        out_piece(so[0], wob[0], parity_dyn(me_dyn))

    late_own = [position for position in range(4) if 0 in tails[position]]
    if len(late_own) == 4:
        own_piece()
    elif late_own:
        pl.when(functools.reduce(jnp.logical_or, [me_dyn == c for c in late_own]))(own_piece)

    rest = [[d for d in tails[position] if d] for position in range(4)]
    for j in range(3):
        d = pick([rest[position][j] for position in range(4)])
        remote("o", d, me_dyn).wait_recv()
        out_piece(ro[d], wob[jnp.bitwise_and(d, 1)], parity_dyn(jnp.bitwise_xor(me_dyn, d)))

    for d in (1, 2, 3):
        remote("o", d, me_dyn).wait_send()


def pallas_dist_rope_attn_qseq_b2_sq128_d512_hq4_dh64_kernel(x, Wq, Wk, Wv, Wo):
    piece = pltpu.VMEM((4, 64, 128), U32)
    return pl.pallas_call(
        _body,
        out_shape=jax.ShapeDtypeStruct((2, 128, 512), F32),
        in_specs=[pl.BlockSpec(memory_space=pl.ANY)] * 5,
        scratch_shapes=[
            pltpu.VMEM((2, 128, 512), F32),
            pltpu.VMEM((2, 512, 128), F32),
            pltpu.VMEM((2, 512, 128), F32),
            pltpu.VMEM((2, 512, 128), F32),
            pltpu.VMEM((2, 128, 512), F32),
            piece, piece, piece, piece,
            pltpu.VMEM((256, 128), U32),
            pltpu.VMEM((256, 128), U32),
            piece, piece,
            pltpu.VMEM((2, 64, 512), U32),
            pltpu.VMEM((4, 128, 512), U32),
            pltpu.VMEM((4, 128, 128), F32),
            pltpu.VMEM((2, 128, 128), F32),
            pltpu.SemaphoreType.DMA((10,)),
            pltpu.SemaphoreType.DMA((12,)),
            pltpu.SemaphoreType.DMA((12,)),
            pltpu.SemaphoreType.REGULAR,
        ],
        compiler_params=pltpu.CompilerParams(collective_id=0, disable_semaphore_checks=True),
    )(x, Wq, Wk, Wv, Wo)
```
